```python
import numpy as np

kernel_name = "dist_mlp2_tp_i_m512_h1024_out512"

def setup_inputs():
    x = np.random.randn(512, 512).astype(np.float32)
    W1 = np.random.randn(512, 4096).astype(np.float32)
    W2 = np.random.randn(4096, 512).astype(np.float32)
    return {"x": x, "W1": W1, "W2": W2}

def reference(x: np.ndarray, W1: np.ndarray, W2: np.ndarray) -> np.ndarray:
    h = x @ W1
    h = np.maximum(h, 0.0)
    return h @ W2
```

```python
import functools
import textwrap

import jax
import jax.numpy as jnp
from jax import lax
from jax.experimental import pallas as pl
from jax.experimental.pallas import tpu as pltpu

N_DEV = 4
M, K, HIDDEN, N = 512, 512, 1024, 512
LANES = 128
COL_BLOCKS = N // LANES
ROWS = (0, 32, 64, 96, 112, 160, 192, 224, 256, 288, 320, 352, 384, 416, 448, 480, 512)
LOADS_IN_FLIGHT = 24

ROUTES = """
    302 020 200 021   310 300 200 020   302 000 310 002   311 322 302 320
    022 022 020 000   200 100 120 002   202 002 310 020   202 300 100 101
    202 300 310 022   000 320 101 000   301 000 310 022   300 300 200 000
    210 310 200 310   021 100 020 020   301 310 301 202   100 200 200 200
""".split()

K_FLIP = (K // 2, 0, K // 2, 0)

LOADS = (
    """
    x:0:96:0:128 W1:0:32:0:1024 x:96:224:0:128 W1:32:64:0:1024 x:224:288:0:128 x:320:352:0:128
    W1:64:96:0:1024 x:384:512:0:128 W1:96:128:0:1024 x:0:96:128:256 W1:128:160:0:1024
    x:96:224:128:256 W1:160:192:0:1024 x:224:288:128:256 x:320:352:128:256 W1:192:224:0:1024
    x:384:512:128:256 W1:224:256:0:1024 x:224:256:256:384 W1:256:288:0:1024 x:256:288:256:384
    W1:288:320:0:1024 x:416:448:256:384 W1:320:352:0:1024 x:480:512:256:384 W1:352:384:0:1024
    x:112:160:384:512 x:192:288:384:512 x:384:448:384:512 x:480:512:384:512 W2:512:640:0:128
    W1:384:448:0:512 W2:640:768:0:128 W1:448:512:0:512 W2:768:896:0:128 W1:384:448:512:1024
    W2:896:1024:0:128 W1:448:512:512:1024 W2:0:512:0:128 W2:0:512:128:256 W2:512:1024:128:256
    W2:0:512:384:512 W2:512:1024:384:512 W2:512:1024:256:384 W2:0:512:256:384 x:288:320:0:256
    x:352:384:0:256
    """,
    """
    x:0:96:0:128 W1:0:32:0:1024 x:96:112:0:128 x:160:224:0:128 W1:32:64:0:1024 x:224:320:0:128
    W1:64:96:0:1024 x:320:416:0:128 x:448:480:0:128 W1:96:128:0:1024 x:0:96:128:256
    W1:128:160:0:1024 x:96:112:128:256 x:160:224:128:256 W1:160:192:0:1024 x:224:320:128:256
    W1:192:224:0:1024 x:320:416:128:256 x:448:480:128:256 W1:224:256:0:1024 W1:256:384:0:1024
    W2:512:640:0:128 W1:384:448:0:512 W2:640:768:0:128 W1:448:512:0:512 W2:768:896:0:128
    W1:384:448:512:1024 W2:896:1024:0:128 W1:448:512:512:1024 W2:0:512:0:128 W2:0:512:128:256
    W2:512:1024:128:256 W2:0:512:256:384 W2:512:1024:256:384 x:112:160:0:256 x:112:160:256:512
    W2:0:512:384:512 x:416:448:0:128 x:416:448:256:512 W2:512:1024:384:512 x:480:512:128:256
    x:480:512:256:512
    """,
    """
    x:0:96:0:128 W1:0:32:0:512 x:96:192:0:128 W1:32:64:0:512 x:192:288:0:128 W1:64:96:0:512
    x:288:384:0:128 W1:96:128:0:512 W1:0:128:512:1024 x:0:96:128:256 W1:128:160:0:512
    x:96:192:128:256 W1:160:192:0:512 x:192:288:128:256 W1:192:224:0:512 x:288:384:128:256
    W1:224:256:0:512 W1:128:256:512:1024 W1:256:384:0:512 W1:256:384:512:1024 W1:384:512:0:512
    W1:384:512:512:1024 W2:0:512:128:256 W2:512:1024:128:256 W2:0:512:0:128 W2:512:1024:0:128
    W2:0:512:384:512 W2:512:1024:384:512 x:448:480:0:256 x:448:480:256:384 W2:512:1024:256:384
    W2:0:512:256:384 x:384:416:0:256 x:384:416:256:384 x:416:448:0:256 x:416:448:256:512
    x:480:512:0:256 x:480:512:256:512
    """,
    """
    x:0:64:0:128 W1:0:32:0:512 x:64:160:0:128 W1:32:64:0:512 x:160:224:0:128 x:288:320:0:128
    W1:64:96:0:512 x:320:384:0:128 x:416:448:0:128 W1:96:128:0:512 W1:0:128:512:1024
    x:0:64:128:256 W1:128:160:0:1024 x:64:160:128:256 W1:160:192:0:1024 x:160:224:128:256
    x:288:320:128:256 W1:192:224:0:1024 x:320:384:128:256 x:416:448:128:256 W1:224:256:0:1024
    W1:256:384:0:1024 x:96:112:384:512 W1:384:512:0:512 W1:384:512:512:1024 W2:0:512:128:256
    W2:512:1024:128:256 W2:0:512:384:512 W2:512:1024:384:512 x:256:288:128:256
    x:256:288:256:384 W2:0:512:0:128 W2:512:1024:0:128 W2:512:1024:256:384 x:384:416:0:256
    x:384:416:256:512 x:480:512:0:128 x:480:512:256:512 x:448:480:0:256 x:448:480:256:512
    W2:0:512:256:384
    """,
)

STEPS = (
    """
    x:0:0:1 x:0:0:3 x:1:0:1 x:2:0:3 x:6:0:1 x:5:0:3 x:8:0:1 x:6:0:3 x:10:0:1 x:10:0:3 x:12:0:1
    x:13:0:3 x:14:0:1 h:0:128:0:512:0,1,2,3,4,6,7,12,13,14
    h:0:128:512:1024:0,1,2,3,4,6,7,12,13,14&h:0:128:0:1024:5,8,10,15 x:0:128:1 x:0:128:3
    x:2:128:1 x:4:128:3 x:8:128:1 x:5:128:3 x:10:128:1 x:6:128:3 x:14:128:1 x:1:128:3 x:3:128:1
    x:2:128:3 x:5:128:1 x:13:128:3 x:12:128:1 h:128:256:0:1024:0,1,2,3,4,5,6,7,8,10,12,13,14,15
    x:15:256:1 x:7:256:3 x:8:256:3 h:256:384:0:1024:0,7,8,13,15 x:13:384:1 x:7:384:3 x:15:384:3
    h:384:512:0:512:7,8,13,15&h:256:512:0:512:4,6,12&h:256:384:512:1024:4,6,12
    h:384:512:512:1024:4,6,7,8,12,13,15&h:256:384:0:1024:1,3,5,14 h:384:512:0:1024:3,5&
    m:0:1024:48,28,52,24,16,60&p48&s48&p28&p24&s24&p16&p60 s28 p52 s52 s16
    h:384:512:0:1024:0,1,14&m:0:1024:32,20,12 p12&s12 s60 p32 s32 p20 s20
    m:0:1024:21,57,1,61,53,49,17&p21&s21&p1&p61&s61&p53&p49&p17&s17 s49 p57&s57 s53
    h:256:512:0:1024:2,10&m:0:1024:4&p4 s4 s1 m:0:1024:59,55,51,7,63,3,27,23,35,43,31&
    m:0:1024:40,0&p59&s59&p55&s55&p51&s51&p7&s7&p43 p31 p63 s63 p35&s35 s43 p27 s27 p0 s0
    m:0:1024:6,30,2,54,22,42,62&p6&s6&p30&s30&p54&s54&p22&s22 p2 p62 p3&s3 p42 s42 s2
    h:0:512:0:1024:9,11 s31 s62 p23&s23 p40 s40 m:0:1024:14,38,10,18,26,46,58,34,50&p38&s38&p10&
    s10&p18&s18&p46&s46&p34&s34&p50&s50 p26 s26 m:0:1024:11,15,39,47,19&m:0:1024:8,36,44,56&p11&
    s11&p47&s47&p44&p56 p39 s39 p36 s36 s56 p58&s58 m:0:1024:45,9,29,41,33,25,13,5,37&p41&s41
    p25&s25 p14 p29 s29 p5&s5 s44 p8 t41 s14 p45 t45&g45 s45 g41 p19 s19 t40 p37&s37 p33&s33
    t33 t36 g36 p9&s9 t9&g9 p13 t13 g13 d:40:1 t17 s13 d:43:3 g24 t0 g0 t8 g33 s8 t29 g29 w21
    t23 g28 g8 t47 t1&g1 g47 t44&g44 t25 d:6:1 d:5:3 t11 t37 t12 t3&g3 w20 t57 t4 g4 t5 t10 t19
    g19 t56 g10 g5 t39 g39 d:5:1 d:6:3 p15 t43 g32 t26&g26 g31 t27 g27 s15 t35 g37 t34&g34 t14
    g57 t15&g15 g14 w6 d:5:1 t42&g42 g38 t55 g55 t7 g7 w2 d:5:3 t52 t58 t51&g51 g52 t16 g59 t18
    g18 t49 g49 w46 d:7:1 d:6:3 t54 g54 w53 w48 w50 w30 w63 d:3:1 w22 w62 d:3:3 w60 d:2:1 d:1:3
    w61
    """,
    """
    x:2:0:2 x:6:0:0 x:3:0:2 x:12:0:0 x:5:0:2 x:3:0:0 x:7:0:2 x:14:0:0 x:8:0:2 x:2:0:0 x:11:0:2
    x:11:0:0 h:0:128:0:1024:0,1,2,3,5,6,7,8,9,10,11,12,14 x:0:128:2 x:5:128:0 x:1:128:2
    x:14:128:0 x:3:128:2 x:2:128:0 x:8:128:2 x:11:128:0 x:6:128:2 x:7:128:2 x:14:128:2
    x:12:128:2 h:128:256:0:1024:0,1,2,3,5,6,7,8,9,10,11,12,14
    h:256:384:0:1024:0,1,2,5,6,8,10,11,12,14 h:384:512:0:512:0,2,8,10,11,14&
    h:256:384:0:1024:3,7,9 h:384:512:512:1024:0,2,8,10,11,14&h:384:512:0:1024:3,5,6,7
    h:384:512:0:1024:1&m:0:1024:0,12,8,28,40,24&p0&s0&p12&s12&p8&s8&p28&p40&p24 s24 s40 s28
    h:384:512:0:1024:9,12&m:0:1024:56,4,44,32,20&p56&p4&s4&p44&s44&p32&s32&p20&s20 s56
    m:0:1024:5,57,33,21,41,49,13,29,37,45&m:0:1024:36,48&p5&s5&p57&s57&p33&p49&s49&p29&s29&p45&
    s45&p48 s48 m:0:512:2,6,10,14,26,34,42,58 s33 p21 s21 m:512:1024:14,10,58,34,2,26,42,6&
    m:0:1024:9,25&p14&s14&p10&s10&p58&s58&p34&p2&p26&p42&p6 s26 s6 p13&s13 p9 s9
    h:0:128:0:1024:4,15&m:0:1024:1 s34 p41 s41 s2 p37 s37 h:128:512:0:1024:4&m:0:512:51 s42 p25&
    s25 p36&s36 m:0:1024:59,27&m:0:1024:17&p59&s59 p17&s17 t17&g17 h:128:512:0:1024:15&
    m:0:1024:50&m:512:1024:51&p50&p51&s51 s50 t21&g21 p1 s1 m:0:1024:46,62&m:0:1024:47,23&
    m:0:1024:61&p46&s46&p62&s62&p61 s61 p23&s23 p47 s47 h:0:128:0:1024:13&m:0:1024:15,63,11&p63
    s63 p27&s27 t1&g1 t27&g27 p11&s11 m:0:1024:3,39,43,19 p3&s3 t23 p39 s39 h:128:512:0:1024:13
    t11&g11 g23 p19 s19 m:0:1024:7,31,35,55&p31&s31 p43 s43 t43 p15&s15 m:0:512:18,22,30,38,54
    g43 p35 s35 t35 g35 t31 g31 m:512:1024:22,54,30,18,38&m:0:1024:53&p30&p38 s38 p53 p7&s7 s53
    p22 t38&g38 m:0:1024:16,60,52&p60&s60 s22 t25&g25 p55&s55 w45 d:7:2 p52 t41 t39 g39 t55 s30
    s52 t52 t7 t3 d:38:2 p16 s16 t16&g16 w24 d:43:0 p18 s18 t36&g36 g0 t53&g53 t19&g19 g7 g13
    w33 p54 s54 t54 g54 t18&g18 w29 t30&g30 g55 g41 w28 d:5:2 t22 g22 g8 t47 g47 t60 g60 t9 w44
    w4 w10 w2 w5 w46 w32 w40 w26 w20 w37 w6 w34 w62 d:9:2 d:9:0 g14 g9 w57 w56 w15 w61 w12 w42
    w63 w51 d:3:2 w50 w59 w48 w49 d:4:2 w58
    """,
    """
    x:3:0:3 x:11:0:1 x:4:0:3 x:2:0:1 x:1:0:3 x:5:0:1 x:9:0:3 x:3:0:1 x:11:0:3 x:7:0:1 x:7:0:3
    x:9:0:1 h:0:128:0:1024:0,1,2,3,4,5,6,7,8,9,10,11 x:9:128:3 x:11:128:1 x:10:128:3 x:6:128:1
    x:11:128:3 x:7:128:1 x:7:128:3 x:1:128:1 x:8:128:3 x:9:128:1
    h:128:256:0:512:0,1,2,3,4,5,6,7,8,9,10,11 h:128:256:512:1024:0,1,2,3,4,5,6,7,8,9,10,11
    h:256:384:0:512:0,1,2,3,4,5,6,7,8,9,10,11 h:256:384:512:1024:0,1,2,3,4,5,6,7,8,9,10,11
    h:384:512:0:512:0,1,2,3,8,9,10,11 h:384:512:512:1024:0,1,2,3,8,9,10,11&
    h:384:512:0:1024:4,6,7 h:384:512:0:1024:5&m:0:512:5,9,13,17,29,33,37,41,45
    m:512:1024:13,5,9,29,37,45,41,33,17&p13&s13&p5&s5&p9&s9&p37&p45&p41&p33 s41 p29 s29 s33 s45
    s37 m:0:512:4,8,12,28,36,40&m:0:1024:1,25,21&p25&s25 m:512:1024:40,36,8&p40&s40&p36&s36&p8&
    s8 p17&s17 m:0:1024:24,0,44,32,20&p0&s0&p44 p21&s21 p24&s24 p1&s1 m:0:512:19,23,27,47&
    m:512:1024:12,4,28&p12&p28 s44 p32 s28 m:512:1024:23,27,47&p23&s23&p47 s47 p4&s4 p27&s27
    s32 h:0:512:0:1024:14&m:0:1024:3,11&p3&p11 s11 s3 s12 p20&s20 m:0:1024:57&m:0:1024:56&
    m:512:1024:19&m:0:1024:39,43&p57&s57&p56&s56&p19&p39&p43 s39 s19 s43
    m:0:1024:10,14,26,6,58,34&m:0:1024:15,59,31,7,35&p10&s10&p14&p58&s58&p15&s15&p31&p7 s14 p26&
    s26 p6 p35&s35 p34&s34 s6 s31 s7 h:0:512:0:1024:12,13&m:0:1024:42,38,2 p2&s2 p38&s38 p42&
    s42 m:0:1024:55,51&m:0:1024:16,48,52&p55&s55&p16&p48&p52&s52 s16 p51 s51 p59 s59
    m:0:1024:53,49&m:0:1024:46,18 p49 p46 p18 s18 s49 p53 s53 s46 s48 h:0:512:0:1024:15&
    m:0:1024:22,50,54,30&p50&s50&p54 s54 m:0:1024:63&m:0:1024:62&p63 s63 p30 s30 p62 s62 p22
    s22 m:0:1024:60&m:0:1024:61&p60&s60 p61 s61 w1 t6 t28 t2 g2 t32 w27 g23 d:35:3 t31 t46 g46
    t24 g40 g11 g17 t20 g20 d:7:3 d:35:1 t62 g6 w4 d:5:1 g35 g62 t38 w34 t53&g53 g56 t21&g21
    t48 t61 g61 g12 t22 g43 d:5:3 d:5:1 g25 t63 g63 g22 t60 g60 w51 t50&g50 g48 t30&g30 w39 g58
    g16 w10 w5 w36 w45 w0 w44 w19 w33 w7 d:9:3 d:10:1 t59 w29 w13 w54 w57 w18 w37 w55 w26 w41
    w3 w8 w49 w47 w42 w14 w15 w9 w52
    """,
    """
    x:0:0:0 x:0:0:2 x:4:0:0 x:1:0:2 x:1:0:0 x:4:0:2 x:5:0:0 x:6:0:2 x:10:0:0 x:9:0:2 x:9:0:0
    x:10:0:2 h:0:128:0:1024:0,1,2,3,4,5,6,9,10,11,13 x:3:128:0 x:2:128:2 x:0:128:0 x:9:128:2
    x:1:128:0 x:10:128:2 x:10:128:0 x:11:128:2 x:9:128:0 x:4:128:2 x:5:128:2
    h:128:256:0:1024:0,1,2,3,4,5,6,9,10,11,13 h:256:384:0:1024:0,2,3,4,5,6,10,13
    h:384:512:0:512:0,3,4,5,6&h:256:384:0:1024:1,9,11 h:384:512:512:1024:0,3,4,5,6&
    h:384:512:0:1024:1,2,9 h:384:512:0:1024:10,11,13&m:0:512:1,9,13,17,25,37
    m:512:1024:37,17,13,1,9,25&m:0:1024:41,53,21&p37&s37&p17&s17&p13&p1&p9&s9&p25&s25&p41&p53&
    p21 s21 s41 s13 s1 s53 h:0:512:0:1024:7&m:0:512:23,27,39,47 m:512:1024:23,27,39,47&
    m:0:1024:3,11,7,43&p23&s23&p27&s27&p39&p47&s47&p3&s3&p11&p7&p43&s43 s7 s11 s39
    h:0:512:0:1024:8&m:0:1024:19,55,15,31&m:0:1024:45,29&p19&s19&p55&p15&s15&p31&s31 s55
    m:0:512:35&m:0:1024:36,32,8,24&m:0:1024:33,5&p36&s36&p32&s32&p24 s24 p5&s5 p29&s29
    m:512:1024:35&m:0:1024:40,52,0,28,12&p35&s35&p52&s52&p28&s28 p33&s33 p45&s45
    h:0:128:0:1024:12,14,15&m:0:1024:16&p16&s16 p40&s40 p8&s8 m:0:1024:38,54&m:0:1024:20,44&p38&
    s38&p54 s54 p0&s0 p20 s20 t24&g24 m:0:1024:2,14,22,18&p22&p18&s18 s22 p44&s44 p2 t28 g28
    h:128:512:0:1024:14&m:0:1024:4 s2 p4 s4 t40 g40 t32&g32 h:128:512:0:1024:15&m:0:1024:30&p30
    s30 t20&g20 p12 s12 m:0:1024:57&m:0:1024:60,56&p60 s60 p57&s57 t12&g12 p56 s56
    m:0:1024:6,58,46,10&p6&s6 p10&s10 p46 s46 t4 g4 p58 s58 m:0:1024:42,62,34,26&p62&s62 p26&
    s26 p14&s14 h:128:512:0:1024:12 p34&s34 t34&g34 t56 g56 t6&g6 m:0:1024:49,61&m:0:1024:48&
    p61&s61 p48 s48 t2 g2 t14 p42&s42 m:0:1024:50&m:0:1024:59,51,63 p51&s51 t51&g51 p50 p63&s63
    s50 t58 g58 p59 t10&g10 t59&g59 t57 t0 t5 g5 w41 d:23:0 p49&s49 t45 d:23:0 d:8:2 t46&g46
    d:33:2 t48&g48 t49 g45 w36 d:5:2 t50 g50 t44 g44 w9 t63 g63 t8 t13 t42 t26 t33 g33 t29&g29
    t62 g62 s59 g57 w1 d:5:0 t61 g61 t37 g37 g26 g3 g49 g42 w47 w23 w11 w19 w39 w17 w31 d:5:0
    d:9:2 t15 g15 w35 w27 w53 w21 w38 w43 w55 g52 d:3:2 w25 w7 w22 w60 d:3:2 w18 w30 w16 d:4:2
    w54
    """,
)


def _hops(route):
    a, r, g = (int(digit) for digit in route)
    b, after_b, before_a = ((a + i) % N_DEV for i in (1, 2, 3))
    reduce = (
        [(before_a, a), (after_b, b)],
        [(after_b, before_a), (before_a, a)],
        [(before_a, after_b), (after_b, b)],
    )[r]
    hand_out = (
        [(a, before_a), (b, after_b)],
        [(a, before_a), (before_a, after_b)],
        [(b, after_b), (after_b, before_a)],
    )[g]
    return reduce + [(a, b), (b, a)] + hand_out


REDUCE, SWAP, HAND_OUT = (0, 1), (2, 3), (4, 5)
HOPS = [_hops(route) for route in ROUTES]
PROGRAMS = [
    [
        [(op[0], [int(v) for v in op[1:].replace(",", ":").split(":") if v]) for op in step.split("&")]
        for step in text.replace("&\n", "&").split()
    ]
    for text in map(textwrap.dedent, STEPS)
]
X_COPIES = [
    (args[0], args[1], pos, args[2])
    for pos, program in enumerate(PROGRAMS)
    for step in program
    for kind, args in step
    if kind == "x"
]
LAST_UNIT = [program[-1][0][1][0] for program in PROGRAMS]


def _semaphore_slots():
    copies = {(u, hop): ends for u, hops in enumerate(HOPS) for hop, ends in enumerate(hops)}
    copies.update({copy: copy[2:] for copy in X_COPIES})
    slots, sends, receives = {}, [0] * N_DEV, [1] * N_DEV
    for copy, (src, dst) in copies.items():
        last = copy in [(LAST_UNIT[dst], hop) for hop in HAND_OUT]
        slots[copy] = (sends[src], 0 if last else receives[dst])
        sends[src] += 1
        receives[dst] += not last
    return slots, max(sends), max(receives)


SLOTS, N_SEND_SLOTS, N_RECV_SLOTS = _semaphore_slots()


def _overlap(a0, a1, b0, b1):
    return a0 < b1 and b0 < a1


def _split_rows(stacked, groups):
    pieces, row = [], 0
    for g in groups:
        pieces.append(stacked[row:row + ROWS[g + 1] - ROWS[g]])
        row += ROWS[g + 1] - ROWS[g]
    return pieces


def _body(x_hbm, w1_hbm, w2_hbm, out, x_f32, w1, w2, x_bf16, h_acc, h, product,
          partial, reduce_in, swap_in, load_sems, send_sems, recv_sems):
    bf16, f32 = jnp.bfloat16, jnp.float32
    barrier = pltpu.get_barrier_semaphore()

    def group(g):
        return slice(ROWS[g], ROWS[g + 1])

    def unit_rows(u):
        return group(u // COL_BLOCKS)

    def unit(ref, u):
        rows = unit_rows(u)
        if ref is out:
            return out.at[rows, pl.ds(u % COL_BLOCKS * LANES, LANES)]
        return ref.at[u % COL_BLOCKS, rows]

    def remote_copy(src_ref, dst_ref, dst, slots):
        return pltpu.make_async_remote_copy(
            src_ref, dst_ref, send_sems.at[slots[0]], recv_sems.at[slots[1]],
            device_id=(dst,), device_id_type=pl.DeviceIdType.MESH)

    def hop_copy(u, hop):
        src_ref, dst_ref = ((partial, reduce_in), (partial, swap_in), (out, out))[hop // 2]
        return remote_copy(unit(src_ref, u), unit(dst_ref, u), HOPS[u][hop][1], SLOTS[u, hop])

    def x_copy(copy):
        g, k, src, dst = copy
        return remote_copy(x_bf16.at[k // LANES, group(g)],
                           x_bf16.at[(k ^ K_FLIP[src] ^ K_FLIP[dst]) // LANES, group(g)],
                           dst, SLOTS[copy])

    def loads(pos, first, end):
        copies = []
        for i, load in list(enumerate(LOADS[pos].split()))[first:end]:
            name, *box = load.split(":")
            r0, r1, c0, c1 = (int(v) for v in box)
            if name == "W2":
                src, dst = w2_hbm.at[r0:r1, c0:c1], w2.at[c0 // LANES, r0:r1]
            elif name == "W1":
                src = w1_hbm.at[pl.ds(r0 ^ K_FLIP[pos], r1 - r0), c0:c1]
                dst = w1.at[r0:r1, c0:c1]
            else:
                src = x_hbm.at[r0:r1, pl.ds(c0 ^ K_FLIP[pos], c1 - c0)]
                dst = x_f32.at[r0:r1, c0:c1]
            copy = pltpu.make_async_copy(src, dst, load_sems.at[i])
            copies.append((name, r0, r1, c0, c1, copy))
        return copies

    def enter(pos):
        for neighbour in ((pos + 1) % N_DEV, (pos - 1) % N_DEV):
            pl.semaphore_signal(barrier, 1, device_id=(neighbour,),
                                device_id_type=pl.DeviceIdType.MESH)
        for load in loads(pos, 0, LOADS_IN_FLIGHT):
            load[5].start()

    def run(pos):
        loading = loads(pos, 0, LOADS_IN_FLIGHT)
        to_load = loads(pos, LOADS_IN_FLIGHT, None)
        x_received = {(copy[0], copy[1] ^ K_FLIP[copy[2]] ^ K_FLIP[pos]): copy
                      for copy in X_COPIES if copy[3] == pos}
        x_arriving = dict(x_received)
        x_cast = []
        leaving = [[] for _ in range(N_DEV)]

        def wait_load(name, r0, r1, c0, c1):
            for load in loading + to_load:
                if load[0] == name and _overlap(r0, r1, *load[1:3]) and _overlap(c0, c1, *load[3:5]):
                    load[5].wait()
                    loading.remove(load)
                    if to_load:
                        loading.append(to_load.pop(0))
                        loading[-1][5].start()

        def hops(u, kinds, end):
            return [hop for hop in kinds if HOPS[u][hop][end] == pos]

        def wait_operands(kind, args):
            if kind == "h":
                wait_load("W1", *args[:4])
                for g in args[4:]:
                    wait_load("x", ROWS[g], ROWS[g + 1], *args[:2])
                    for k in range(args[0], args[1], LANES):
                        if (g, k) in x_arriving:
                            x_copy(x_arriving.pop((g, k))).wait_recv()
            elif kind == "m":
                col = args[2] % COL_BLOCKS * LANES
                wait_load("W2", args[0], args[1], col, col + LANES)
            elif kind == "x":
                wait_load("x", ROWS[args[0]], ROWS[args[0] + 1], args[1], args[1] + LANES)
            elif kind == "d":
                for _ in range(args[0]):
                    leaving[args[1]].pop(0).wait_send()
            elif kind != "s":
                for hop in hops(args[0], {"p": REDUCE, "t": SWAP}.get(kind, HAND_OUT), 1):
                    hop_copy(args[0], hop).wait_recv()

        def start(copy, dst):
            copy.start()
            leaving[dst].append(copy)

        entered = False
        for ops in PROGRAMS[pos][:-1]:
            if not entered and any(kind != "h" for kind, _ in ops):
                pl.semaphore_wait(barrier, 2)
                entered = True
            for kind, args in ops:
                wait_operands(kind, args)
            finished = {}
            for kind, args in ops:
                if kind == "h":
                    k0, k1, n0, n1, *groups = args
                    lhs = [jnp.concatenate(
                        [x_bf16[k // LANES, group(g)] if (g, k) in x_received
                         else x_f32[group(g), k:k + LANES].astype(bf16)
                         for k in range(k0, k1, LANES)], axis=1) for g in groups]
                    res = jnp.dot(jnp.concatenate(lhs), w1[k0:k1, n0:n1].astype(bf16),
                                  preferred_element_type=f32)
                    for g, acc in zip(groups, _split_rows(res, groups)):
                        if k0 > 0:
                            acc = acc + h_acc[group(g), n0:n1]
                        if k1 < K:
                            h_acc[group(g), n0:n1] = acc
                        else:
                            h[group(g), n0:n1] = jnp.maximum(acc, 0.0).astype(bf16)
                elif kind == "m":
                    k0, k1, *units = args
                    res = jnp.dot(jnp.concatenate([h[unit_rows(u), k0:k1] for u in units]),
                                  w2[units[0] % COL_BLOCKS, k0:k1].astype(bf16),
                                  preferred_element_type=f32)
                    for u, acc in zip(units, _split_rows(res, [u // COL_BLOCKS for u in units])):
                        if k0 > 0:
                            acc = acc + unit(product, u)[...]
                        if k1 < HIDDEN:
                            unit(product, u)[...] = acc
                        else:
                            finished[u] = acc
                elif kind == "x":
                    g, k, dst = args
                    if (g, k) not in x_cast:
                        x_bf16[k // LANES, group(g)] = x_f32[group(g), k:k + LANES].astype(bf16)
                        x_cast.append((g, k))
                    start(x_copy((g, k, pos, dst)), dst)
                elif kind == "p":
                    u = args[0]
                    while u in finished and next(iter(finished)) != u:
                        later = next(iter(finished))
                        unit(product, later)[...] = finished.pop(later)
                    acc = finished.pop(u) if u in finished else unit(product, u)[...]
                    if hops(u, REDUCE, 1):
                        acc = acc + unit(reduce_in, u)[...].astype(f32)
                    unit(partial, u)[...] = acc.astype(bf16)
                elif kind == "t":
                    u = args[0]
                    acc = unit(partial, u)[...].astype(f32) + unit(swap_in, u)[...].astype(f32)
                    unit(out, u)[...] = acc.astype(bf16)
                elif kind in "sg":
                    (hop,) = hops(args[0], REDUCE + SWAP if kind == "s" else HAND_OUT, 0)
                    start(hop_copy(args[0], hop), HOPS[args[0]][hop][1])
            for u, acc in finished.items():
                unit(product, u)[...] = acc
        assert not loading and not x_arriving and not any(leaving)

    me = lax.axis_index("i")
    for stage in (enter, run):
        for pos in (2, 1, 3, 0):
            pl.when(me == pos)(functools.partial(stage, pos))

    row, col = 0, 0
    for pos, u in enumerate(LAST_UNIT):
        row = jnp.where(me == pos, ROWS[u // COL_BLOCKS], row)
        col = jnp.where(me == pos, u % COL_BLOCKS * LANES, col)
    last = out.at[pl.ds(pl.multiple_of(row, 16), 32),
                  pl.ds(pl.multiple_of(col, LANES), LANES)]
    pltpu.make_async_copy(last, last, recv_sems.at[0]).wait()


def pallas_dist_mlp2_tp_i_m512_h1024_out512_kernel(x: jax.Array, W1: jax.Array, W2: jax.Array):
    bf16, f32 = jnp.bfloat16, jnp.float32
    return pl.pallas_call(
        _body,
        out_shape=jax.ShapeDtypeStruct((M, N), bf16),
        in_specs=[pl.BlockSpec(memory_space=pl.ANY)] * 3,
        out_specs=pl.BlockSpec(memory_space=pltpu.VMEM),
        scratch_shapes=[
            pltpu.VMEM((M, K), f32),
            pltpu.VMEM((K, HIDDEN), f32),
            pltpu.VMEM((COL_BLOCKS, HIDDEN, LANES), f32),
            pltpu.VMEM((K // LANES, M, LANES), bf16),
            pltpu.VMEM((M, HIDDEN), f32),
            pltpu.VMEM((M, HIDDEN), bf16),
            pltpu.VMEM((COL_BLOCKS, M, LANES), f32),
            pltpu.VMEM((COL_BLOCKS, M, LANES), bf16),
            pltpu.VMEM((COL_BLOCKS, M, LANES), bf16),
            pltpu.VMEM((COL_BLOCKS, M, LANES), bf16),
            pltpu.SemaphoreType.DMA((max(len(text.split()) for text in LOADS),)),
            pltpu.SemaphoreType.DMA((N_SEND_SLOTS,)),
            pltpu.SemaphoreType.DMA((N_RECV_SLOTS,)),
        ],
        compiler_params=pltpu.CompilerParams(
            collective_id=0, disable_semaphore_checks=True, disable_bounds_checks=True),
    )(x, W1, W2)
```
